```python
import numpy as np

kernel_name = "dist_sum_ax1_xy_m512_n256"

def setup_inputs():
    return {"x": np.random.randn(1024, 512).astype(np.float32)}

def reference(x: np.ndarray) -> np.ndarray:
    return np.sum(x, axis=1, keepdims=True)
```

```python
import jax
import jax.numpy as jnp
from jax import lax
from jax.experimental import pallas as pl
from jax.experimental.pallas import tpu as pltpu

_LANES = 128
_SUBLANES = 8
_RAW_ROWS = 16
_CHUNK_ENDS = (128, 256, 384, 408, 432, 456, 480, 496, 512)
_EARLY = 384


def _kernel(
    x_ref,
    o_ref,
    xv,
    raw,
    head,
    early_mine,
    early_theirs,
    late_mine,
    late_theirs,
    staged,
    ordered,
    load_sems,
    local_sem,
    send_sems,
    recv_sems,
):
    starts = (_RAW_ROWS,) + _CHUNK_ENDS[:-1]
    loads = [
        pltpu.make_async_copy(
            x_ref.at[pl.ds(lo, hi - lo)], xv.at[pl.ds(lo, hi - lo)], load_sems.at[i]
        )
        for i, (lo, hi) in enumerate(zip(starts, _CHUNK_ENDS))
    ]
    for load in loads[:-1]:
        load.start()
    loads[-1].start(priority=1)

    my_y = lax.axis_index("y")
    peer = (lax.axis_index("x"), 1 - my_y)
    barrier = pltpu.get_barrier_semaphore()
    pl.semaphore_signal(
        barrier, inc=1, device_id=peer, device_id_type=pl.DeviceIdType.MESH
    )

    def remote_copy(src, dst, i):
        return pltpu.make_async_remote_copy(
            src,
            dst,
            send_sems.at[i],
            recv_sems.at[i],
            device_id=peer,
            device_id_type=pl.DeviceIdType.MESH,
        )

    first_rows = x_ref.at[pl.ds(0, _RAW_ROWS)]
    send_raw = remote_copy(first_rows, raw, 0)
    send_early = remote_copy(early_mine, early_theirs, 1)
    send_late = remote_copy(late_mine, late_theirs, 2)

    lane = lax.broadcasted_iota(jnp.int32, (_SUBLANES, _LANES), 1)
    zeros = jnp.zeros((_SUBLANES, _LANES), jnp.float32)

    def reduce_rows(block, ref, lo, hi):
        for r in range(lo, hi, _SUBLANES):
            rows = pl.ds(r, _SUBLANES)
            halves = ref[rows, :_LANES] + ref[rows, _LANES:]
            sums = jnp.broadcast_to(jnp.sum(halves, axis=1, keepdims=True), zeros.shape)
            group = r % _LANES // _SUBLANES
            block = (
                sums if block is None else jnp.where(lane >> 3 == group, sums, block)
            )
        return block

    def lane_major(block):
        return jnp.take_along_axis(block, lane & 7, axis=0)[:1]

    def finish(src):
        copy = pltpu.make_async_copy(src, ordered, local_sem)
        copy.start()
        copy.wait()

    @pl.when(my_y == 1)
    def _():
        pl.semaphore_wait(barrier, 1)
        send_raw.start()

    head[...] = zeros

    @pl.when(my_y == 0)
    def _():
        copy = pltpu.make_async_copy(
            first_rows, xv.at[pl.ds(0, _RAW_ROWS)], local_sem
        )
        copy.start()
        copy.wait()
        head[...] = reduce_rows(zeros, xv, 0, _RAW_ROWS)
        pl.semaphore_wait(barrier, 1)

    mine = []
    block = head[...]
    for load, lo, hi in zip(loads, starts, _CHUNK_ENDS):
        load.wait()
        block = reduce_rows(block, xv, lo, hi)
        if hi % _LANES:
            continue
        mine.append(lane_major(block))
        block = None
        if hi > _EARLY:
            late_mine[...] = mine[-1]
            send_late.start()
            continue
        lanes = pl.ds(hi - _LANES, _LANES)
        early_mine[:, lanes] = mine[-1]
        if hi == _EARLY:
            send_early.start()
        else:
            finish(early_mine.at[:, lanes])

    send_early.wait_send()
    send_late.wait_send()

    @pl.when(my_y == 1)
    def _():
        send_raw.wait_send()
        copy = pltpu.make_async_copy(first_rows, raw, local_sem)
        copy.start()
        copy.wait()

    @pl.when(my_y == 0)
    def _():
        send_raw.wait_recv()

    staged[...] = mine[0] + lane_major(reduce_rows(zeros, raw, 0, _RAW_ROWS))
    finish(staged)
    mine[0] = ordered[...]

    send_early.wait_recv()
    for i in range(_EARLY // _LANES):
        lanes = pl.ds(i * _LANES, _LANES)
        o_ref[:, lanes] = mine[i] + early_theirs[:, lanes]
    send_late.wait_recv()
    o_ref[:, pl.ds(_EARLY, _LANES)] = mine[-1] + late_theirs[...]


def pallas_dist_sum_ax1_xy_m512_n256_kernel(
    x: jax.Array,
):
    m, n = x.shape
    assert (m, n) == (_EARLY + _LANES, 2 * _LANES)

    def vmem(*shape):
        return pltpu.VMEM(shape, jnp.float32)

    out = pl.pallas_call(
        _kernel,
        out_shape=jax.ShapeDtypeStruct((1, m), x.dtype),
        in_specs=[pl.BlockSpec(memory_space=pltpu.HBM)],
        out_specs=pl.BlockSpec(memory_space=pltpu.VMEM),
        scratch_shapes=[
            vmem(m, n),
            vmem(_RAW_ROWS, n),
            vmem(_SUBLANES, _LANES),
            vmem(1, _EARLY),
            vmem(1, _EARLY),
            vmem(1, _LANES),
            vmem(1, _LANES),
            vmem(1, _LANES),
            vmem(1, _LANES),
            pltpu.SemaphoreType.DMA((len(_CHUNK_ENDS),)),
            pltpu.SemaphoreType.DMA,
            pltpu.SemaphoreType.DMA((3,)),
            pltpu.SemaphoreType.DMA((3,)),
        ],
        compiler_params=pltpu.CompilerParams(
            collective_id=0,
            disable_bounds_checks=True,
            disable_semaphore_checks=True,
            flags={"XLA_TPU_RESCHEDULE_DMA_DONES": True},
        ),
    )(x)
    return out.reshape(m, 1)
```

```python
import jax
import jax.numpy as jnp
from jax import lax
from jax.experimental import pallas as pl
from jax.experimental.pallas import tpu as pltpu

_LANES = 128
_SUBLANES = 8
_EARLY = 384
_HANDED_OVER = ((104, 128), (504, 512))
_LOADED = (
    (0, 104),
    (128, 256),
    (256, 384),
    (384, 424),
    (424, 448),
    (448, 464),
    (464, 480),
    (480, 488),
    (488, 504),
)
_SECOND_HANDOVER = 1


def _kernel(
    x_ref,
    o_ref,
    xv,
    handed,
    seeds,
    mine,
    theirs,
    sink,
    load_sems,
    range_sems,
    send_sems,
    recv_sems,
):
    def rows(ref, lo, hi):
        return ref.at[pl.ds(lo, hi - lo)]

    loads = [
        pltpu.make_async_copy(rows(x_ref, *r), rows(xv, *r), load_sems.at[i])
        for i, r in enumerate(_LOADED)
    ]
    for load in loads[:-1]:
        load.start()
    loads[-1].start(priority=1)

    my_y = lax.axis_index("y")
    peer = (lax.axis_index("x"), 1 - my_y)
    barrier = pltpu.get_barrier_semaphore()
    pl.semaphore_signal(
        barrier, inc=1, device_id=peer, device_id_type=pl.DeviceIdType.MESH
    )

    def remote_copy(src, dst, i):
        return pltpu.make_async_remote_copy(
            src,
            dst,
            send_sems.at[i],
            recv_sems.at[i],
            device_id=peer,
            device_id_type=pl.DeviceIdType.MESH,
        )

    early = pl.ds(0, _EARLY)
    late = pl.ds(_EARLY, _LANES)
    send_early = remote_copy(mine.at[:, early], theirs.at[:, early], 0)
    send_late = remote_copy(mine.at[:, late], theirs.at[:, late], 1)
    handovers = [
        remote_copy(rows(x_ref, *r), rows(handed, *r), 2 + i)
        for i, r in enumerate(_HANDED_OVER)
    ]

    def load_handed_over_ranges(dst):
        copies = [
            pltpu.make_async_copy(rows(x_ref, *r), rows(dst, *r), range_sems.at[i])
            for i, r in enumerate(_HANDED_OVER)
        ]
        for copy in copies:
            copy.start()
        for copy in copies:
            copy.wait()

    lane = lax.broadcasted_iota(jnp.int32, (_SUBLANES, _LANES), 1)
    zeros = jnp.zeros((_SUBLANES, _LANES), jnp.float32)

    def reduce_rows(block, ref, lo, hi):
        for r in range(lo, hi, _SUBLANES):
            group = pl.ds(r, _SUBLANES)
            halves = ref[group, :_LANES] + ref[group, _LANES:]
            sums = jnp.broadcast_to(jnp.sum(halves, axis=1, keepdims=True), zeros.shape)
            here = (lane >> 3) == r % _LANES // _SUBLANES
            block = sums if block is None else jnp.where(here, sums, block)
        return block

    def lane_major(block):
        return jnp.take_along_axis(block, lane & 7, axis=0)[:1]

    def finish(lanes, sems):
        copy = pltpu.make_async_copy(
            mine.at[:, lanes], sink, sems.at[sems.shape[0] - 1]
        )
        copy.start()
        copy.wait()

    @pl.when(my_y == 1)
    def _():
        pl.semaphore_wait(barrier, 1)
        handovers[0].start()

    for i in range(len(_HANDED_OVER)):
        seeds[i] = zeros

    @pl.when(my_y == 0)
    def _():
        load_handed_over_ranges(xv)
        for i, r in enumerate(_HANDED_OVER):
            seeds[i] = reduce_rows(zeros, xv, *r)
        pl.semaphore_wait(barrier, 1)

    blocks = {lo // _LANES: seeds[i] for i, (lo, _) in enumerate(_HANDED_OVER)}
    for i, (load, (lo, hi)) in enumerate(zip(loads, _LOADED)):
        load.wait()
        if i == _SECOND_HANDOVER:
            pl.when(my_y == 1)(handovers[1].start)
        b = lo // _LANES
        blocks[b] = reduce_rows(blocks.get(b), xv, lo, hi)
        if i + 1 < len(loads) and _LOADED[i + 1][0] // _LANES == b:
            continue
        lanes = pl.ds(b * _LANES, _LANES)
        mine[:, lanes] = lane_major(blocks[b])
        if (b + 1) * _LANES < _EARLY:
            finish(lanes, load_sems)
        elif (b + 1) * _LANES == _EARLY:
            send_early.start()
        else:
            send_late.start()
    send_early.wait_send()
    send_late.wait_send()

    @pl.when(my_y == 1)
    def _():
        for handover in handovers:
            handover.wait_send()
        load_handed_over_ranges(handed)

    @pl.when(my_y == 0)
    def _():
        for handover in handovers:
            handover.wait_recv()

    extras = [lane_major(reduce_rows(zeros, handed, *r)) for r in _HANDED_OVER]
    for (lo, _), extra in zip(_HANDED_OVER, extras):
        b = lo // _LANES
        lanes = pl.ds(b * _LANES, _LANES)
        mine[:, lanes] = lane_major(blocks[b]) + extra
        finish(lanes, recv_sems)

    total = mine[...]
    send_early.wait_recv()
    send_late.wait_recv()
    o_ref[...] = total + theirs[...]


def pallas_dist_sum_ax1_xy_m512_n256_kernel(
    x: jax.Array,
):
    m, n = x.shape
    assert (m, n) == (_EARLY + _LANES, 2 * _LANES)

    def vmem(*shape):
        return pltpu.VMEM(shape, jnp.float32)

    out = pl.pallas_call(
        _kernel,
        out_shape=jax.ShapeDtypeStruct((1, m), x.dtype),
        in_specs=[pl.BlockSpec(memory_space=pltpu.HBM)],
        out_specs=pl.BlockSpec(memory_space=pltpu.VMEM),
        scratch_shapes=[
            vmem(m, n),
            vmem(m, n),
            vmem(len(_HANDED_OVER), _SUBLANES, _LANES),
            vmem(1, m),
            vmem(1, m),
            vmem(1, _LANES),
            pltpu.SemaphoreType.DMA((len(_LOADED) + 1,)),
            pltpu.SemaphoreType.DMA((len(_HANDED_OVER),)),
            pltpu.SemaphoreType.DMA((2 + len(_HANDED_OVER),)),
            pltpu.SemaphoreType.DMA((2 + len(_HANDED_OVER) + 1,)),
        ],
        compiler_params=pltpu.CompilerParams(
            collective_id=0,
            disable_bounds_checks=True,
            disable_semaphore_checks=True,
            flags={"XLA_TPU_RESCHEDULE_DMA_DONES": True},
        ),
    )(x)
    return out.reshape(m, 1)
```
